```python
import numpy as np

kernel_name = "dist_mean_ax0_shard0_i_m2048_n1024"

def setup_inputs():
    return {"x": np.random.randn(8192, 1024).astype(np.float32)}

def reference(x: np.ndarray) -> np.ndarray:
    return np.mean(x, axis=0, keepdims=True)
```

```python
import jax
import jax.numpy as jnp
from jax import lax
from jax.experimental import pallas as pl
from jax.experimental.pallas import tpu as pltpu

N_DEV = 4
SUBLANES = 8

CHUNK_ROWS = 256
DEPTH = 3


def pallas_dist_mean_ax0_shard0_i_m2048_n1024_kernel(
    x: jax.Array,
):
    m_per, n = x.shape
    assert m_per % CHUNK_ROWS == 0
    n_chunks = m_per // CHUNK_ROWS
    inv_total = 1.0 / float(N_DEV * m_per)

    def kernel_body(x_hbm, out_ref, xbuf, comm, load_sems, send_sems, recv_sems):
        my = lax.axis_index("i")

        barrier_sem = pltpu.get_barrier_semaphore()
        for d in range(1, N_DEV):
            pl.semaphore_signal(
                barrier_sem,
                inc=1,
                device_id=((my + d) % N_DEV,),
                device_id_type=pl.DeviceIdType.MESH,
            )

        def load(c):
            return pltpu.make_async_copy(
                x_hbm.at[pl.ds(c * CHUNK_ROWS, CHUNK_ROWS), :],
                xbuf.at[pl.ds(c * CHUNK_ROWS, CHUNK_ROWS), :],
                load_sems.at[c],
            )

        for c in range(min(DEPTH, n_chunks)):
            load(c).start()

        acc = jnp.zeros((SUBLANES, n), jnp.float32)
        for c in range(n_chunks):
            load(c).wait()
            if c + DEPTH < n_chunks:
                load(c + DEPTH).start()

            def add_rows(r, a, c=c):
                start = pl.multiple_of(c * CHUNK_ROWS + r * SUBLANES, SUBLANES)
                return a + xbuf[pl.ds(start, SUBLANES), :]

            acc = lax.fori_loop(0, CHUNK_ROWS // SUBLANES, add_rows, acc, unroll=8)

        part = jnp.sum(acc, axis=0, keepdims=True)
        comm[0] = part

        pl.semaphore_wait(barrier_sem, N_DEV - 1)

        copies = []
        for d in range(1, N_DEV):
            cp = pltpu.make_async_remote_copy(
                src_ref=comm.at[0],
                dst_ref=comm.at[d],
                send_sem=send_sems.at[d - 1],
                recv_sem=recv_sems.at[d - 1],
                device_id=((my + d) % N_DEV,),
                device_id_type=pl.DeviceIdType.MESH,
            )
            cp.start()
            copies.append(cp)

        total = part
        for d in range(1, N_DEV):
            copies[d - 1].wait_recv()
            total = total + comm[d]
        out_ref[...] = total * inv_total

        for cp in copies:
            cp.wait_send()

    return pl.pallas_call(
        kernel_body,
        out_shape=jax.ShapeDtypeStruct((1, n), jnp.float32),
        in_specs=[pl.BlockSpec(memory_space=pl.ANY)],
        out_specs=pl.BlockSpec(memory_space=pltpu.VMEM),
        scratch_shapes=[
            pltpu.VMEM((m_per, n), jnp.float32),
            pltpu.VMEM((N_DEV, 1, n), jnp.float32),
            pltpu.SemaphoreType.DMA((n_chunks,)),
            pltpu.SemaphoreType.DMA((N_DEV - 1,)),
            pltpu.SemaphoreType.DMA((N_DEV - 1,)),
        ],
        compiler_params=pltpu.CompilerParams(collective_id=0),
    )(x)
```

```python
import jax
import jax.numpy as jnp
from jax import lax
from jax.experimental import pallas as pl
from jax.experimental.pallas import tpu as pltpu

N_DEV = 4
SUB = 8
LANES = 128

ASSIST_ROWS = 96
N_BIG = 2
LOCAL_TAIL = (128, 64, 32)
STAIR_ROWS = 48
STAIR_BLOCKS = (4, 1, 1, 1, 1)
INNER = 4


def pallas_dist_mean_ax0_shard0_i_m2048_n1024_kernel(
    x: jax.Array,
):
    m_per, n = x.shape
    nb = n // LANES
    assert n == nb * LANES and nb == SUB and sum(STAIR_BLOCKS) == nb

    a_rows = ASSIST_ROWS
    l_rows = m_per - 2 * a_rows
    s_row0 = l_rows - STAIR_ROWS
    big = s_row0 - sum(LOCAL_TAIL)
    b0 = (big // N_BIG) // SUB * SUB
    chunks = [b0] * (N_BIG - 1) + [big - b0 * (N_BIG - 1)] + list(LOCAL_TAIL)
    assert all(c > 0 and c % SUB == 0 for c in chunks)
    offs = [0]
    for c in chunks:
        offs.append(offs[-1] + c)
    assert offs[-1] == s_row0
    n_chunks = len(chunks)
    assist_at = N_BIG + 1

    s_off = [0]
    for w in STAIR_BLOCKS:
        assert w & (w - 1) == 0 and s_off[-1] % w == 0
        s_off.append(s_off[-1] + w)
    n_stairs = len(STAIR_BLOCKS)
    inv_total = 1.0 / float(N_DEV * m_per)

    def kernel_body(
        x_hbm,
        out_ref,
        xbuf,
        abuf,
        comm,
        load_sems,
        stair_sems,
        a_send_sems,
        a_recv_sems,
        d_send_sems,
        n_send_sems,
        recv_sems,
    ):
        my = lax.axis_index("i")

        def peer(d):
            return ((my + d) % N_DEV,)

        def load(c):
            rows = pl.ds(offs[c], chunks[c])
            return pltpu.make_async_copy(
                x_hbm.at[rows, :], xbuf.at[rows, :], load_sems.at[c]
            )

        def stair_load(s):
            rows = pl.ds(s_row0, STAIR_ROWS)
            cols = pl.ds(s_off[s] * LANES, STAIR_BLOCKS[s] * LANES)
            return pltpu.make_async_copy(
                x_hbm.at[rows, cols], xbuf.at[rows, cols], stair_sems.at[s]
            )

        for c in range(n_chunks):
            load(c).start()
        for s in range(n_stairs):
            stair_load(s).start()

        barrier_sem = pltpu.get_barrier_semaphore()
        for d in range(1, N_DEV):
            pl.semaphore_signal(
                barrier_sem,
                inc=1,
                device_id=peer(d),
                device_id_type=pl.DeviceIdType.MESH,
            )
        pl.semaphore_wait(barrier_sem, N_DEV - 1)

        assists = []
        for k, d in enumerate((1, N_DEV - 1)):
            cp = pltpu.make_async_remote_copy(
                src_ref=x_hbm.at[pl.ds(l_rows + k * a_rows, a_rows), :],
                dst_ref=abuf.at[pl.ds(k * a_rows, a_rows), :],
                send_sem=a_send_sems.at[k],
                recv_sem=a_recv_sems.at[k],
                device_id=peer(d),
                device_id_type=pl.DeviceIdType.MESH,
            )
            cp.start()
            assists.append(cp)

        def accumulate(ref, row0, nrows, acc):
            groups = nrows // SUB
            trips = groups // INNER if groups > 2 * INNER else 0
            if trips:

                def step(r, a):
                    base = pl.multiple_of(row0 + r * (SUB * INNER), SUB)
                    for u in range(INNER):
                        a = a + ref[pl.ds(base + u * SUB, SUB), :]
                    return a

                acc = lax.fori_loop(0, trips, step, acc)
            for g in range(trips * INNER, groups):
                acc = acc + ref[pl.ds(row0 + g * SUB, SUB), :]
            return acc

        acc = jnp.zeros((SUB, n), jnp.float32)
        for c in range(n_chunks):
            if c == assist_at:
                for k, cp in enumerate(assists):
                    cp.wait_recv()
                    acc = accumulate(abuf, k * a_rows, a_rows, acc)
            load(c).wait()
            acc = accumulate(xbuf, offs[c], chunks[c], acc)

        row = lax.broadcasted_iota(jnp.int32, (SUB, LANES), 0)
        d_copies = []
        for s in range(n_stairs):
            stair_load(s).wait()
            vs = []
            for j in range(s_off[s], s_off[s + 1]):
                cols = slice(j * LANES, (j + 1) * LANES)
                terms = [
                    xbuf[pl.ds(s_row0 + g * SUB, SUB), cols]
                    for g in range(STAIR_ROWS // SUB)
                ]
                terms.append(acc[:, cols])
                while len(terms) > 1:
                    terms = [
                        terms[i] + terms[i + 1] if i + 1 < len(terms) else terms[i]
                        for i in range(0, len(terms), 2)
                    ]
                vs.append(terms[0])
            shift = 1
            while shift < SUB:
                if len(vs) > 1:
                    keep = (row & shift) == 0
                    vs = [
                        jnp.where(keep, vs[2 * j], vs[2 * j + 1])
                        + pltpu.roll(
                            jnp.where(keep, vs[2 * j + 1], vs[2 * j]), shift, 0
                        )
                        for j in range(len(vs) // 2)
                    ]
                else:
                    vs = [vs[0] + pltpu.roll(vs[0], shift, 0)]
                shift *= 2
            packed = vs[0] * inv_total
            rows = pl.ds(s_off[s], STAIR_BLOCKS[s])
            comm[0, rows, :] = packed[s_off[s] : s_off[s + 1], :]
            cp = pltpu.make_async_remote_copy(
                src_ref=comm.at[0, rows],
                dst_ref=comm.at[2, rows],
                send_sem=d_send_sems.at[s],
                recv_sem=recv_sems.at[1],
                device_id=peer(2),
                device_id_type=pl.DeviceIdType.MESH,
            )
            cp.start()
            d_copies.append(cp)

        n_copies = []
        for k, d in enumerate((1, N_DEV - 1)):
            cp = pltpu.make_async_remote_copy(
                src_ref=comm.at[0],
                dst_ref=comm.at[d],
                send_sem=n_send_sems.at[k],
                recv_sem=recv_sems.at[d - 1],
                device_id=peer(d),
                device_id_type=pl.DeviceIdType.MESH,
            )
            cp.start()
            n_copies.append(cp)

        total = comm[0]
        for cp in assists + d_copies + n_copies:
            cp.wait_send()
        for cp, d in zip(n_copies, (1, N_DEV - 1)):
            cp.wait_recv()
            total = total + comm[d]
        pltpu.make_async_copy(comm.at[2], comm.at[2], recv_sems.at[1]).wait()
        out_ref[...] = total + comm[2]

    out = pl.pallas_call(
        kernel_body,
        out_shape=jax.ShapeDtypeStruct((nb, LANES), jnp.float32),
        in_specs=[pl.BlockSpec(memory_space=pl.ANY)],
        out_specs=pl.BlockSpec(memory_space=pltpu.VMEM),
        scratch_shapes=[
            pltpu.VMEM((l_rows, n), jnp.float32),
            pltpu.VMEM((2 * a_rows, n), jnp.float32),
            pltpu.VMEM((N_DEV, nb, LANES), jnp.float32),
            pltpu.SemaphoreType.DMA((n_chunks,)),
            pltpu.SemaphoreType.DMA((n_stairs,)),
            pltpu.SemaphoreType.DMA((2,)),
            pltpu.SemaphoreType.DMA((2,)),
            pltpu.SemaphoreType.DMA((n_stairs,)),
            pltpu.SemaphoreType.DMA((2,)),
            pltpu.SemaphoreType.DMA((N_DEV - 1,)),
        ],
        compiler_params=pltpu.CompilerParams(
            collective_id=0,
            disable_semaphore_checks=True,
            disable_bounds_checks=True,
        ),
    )(x)
    return out.reshape(1, n)
```

```python
import jax
import jax.numpy as jnp
from jax import lax
from jax.experimental import pallas as pl
from jax.experimental.pallas import tpu as pltpu

N_DEV = 4
SUB = 8
LANES = 128

ASSIST_ROWS = 96
N_BIG = 2
LOCAL_TAIL = (128, 64, 32)
STAIR_ROWS = 48
STAIR_BLOCKS = (4, 1, 1, 1, 1)
INNER = 4


def pallas_dist_mean_ax0_shard0_i_m2048_n1024_kernel(
    x: jax.Array,
):
    m_per, n = x.shape
    nb = n // LANES
    assert n == nb * LANES and nb == SUB and sum(STAIR_BLOCKS) == nb

    a_rows = ASSIST_ROWS
    l_rows = m_per - 2 * a_rows
    s_row0 = l_rows - STAIR_ROWS
    big = s_row0 - sum(LOCAL_TAIL)
    b0 = (big // N_BIG) // SUB * SUB
    chunks = [b0] * (N_BIG - 1) + [big - b0 * (N_BIG - 1)] + list(LOCAL_TAIL)
    assert all(c > 0 and c % SUB == 0 for c in chunks)
    offs = [0]
    for c in chunks:
        offs.append(offs[-1] + c)
    assert offs[-1] == s_row0
    n_chunks = len(chunks)
    assist_at = N_BIG + 1

    s_off = [0]
    for w in STAIR_BLOCKS:
        assert w & (w - 1) == 0 and s_off[-1] % w == 0
        s_off.append(s_off[-1] + w)
    n_stairs = len(STAIR_BLOCKS)
    inv_total = 1.0 / float(N_DEV * m_per)
    nbrs = (1, N_DEV - 1)
    diag = 2

    def kernel_body(x_hbm, out_ref, xbuf, abuf, comm):
        def scoped(
            load_sems,
            stair_sems,
            a_send_sems,
            a_recv_sems,
            d_send_sems,
            d_recv_sem,
            n_send_sems,
            n_recv_sems,
        ):
            def load(c):
                rows = pl.ds(offs[c], chunks[c])
                return pltpu.make_async_copy(
                    x_hbm.at[rows, :], xbuf.at[rows, :], load_sems.at[c]
                )

            def stair_load(s):
                rows = pl.ds(s_row0, STAIR_ROWS)
                cols = pl.ds(s_off[s] * LANES, STAIR_BLOCKS[s] * LANES)
                return pltpu.make_async_copy(
                    x_hbm.at[rows, cols], xbuf.at[rows, cols], stair_sems.at[s]
                )

            for c in range(n_chunks):
                load(c).start()
            for s in range(n_stairs):
                stair_load(s).start()

            my = lax.axis_index("i")

            def peer(d):
                return ((my + d) % N_DEV,)

            barrier_sem = pltpu.get_barrier_semaphore()
            for d in range(1, N_DEV):
                pl.semaphore_signal(
                    barrier_sem,
                    inc=1,
                    device_id=peer(d),
                    device_id_type=pl.DeviceIdType.MESH,
                )
            pl.semaphore_wait(barrier_sem, N_DEV - 1)

            assists = []
            for k, d in enumerate(nbrs):
                cp = pltpu.make_async_remote_copy(
                    src_ref=x_hbm.at[pl.ds(l_rows + k * a_rows, a_rows), :],
                    dst_ref=abuf.at[pl.ds(k * a_rows, a_rows), :],
                    send_sem=a_send_sems.at[k],
                    recv_sem=a_recv_sems.at[k],
                    device_id=peer(d),
                    device_id_type=pl.DeviceIdType.MESH,
                )
                cp.start()
                assists.append(cp)

            def accumulate(ref, row0, nrows, acc):
                groups = nrows // SUB
                trips = groups // INNER if groups > 2 * INNER else 0
                if trips:

                    def step(r, a):
                        base = pl.multiple_of(row0 + r * (SUB * INNER), SUB)
                        for u in range(INNER):
                            a = a + ref[pl.ds(base + u * SUB, SUB), :]
                        return a

                    acc = lax.fori_loop(0, trips, step, acc)
                for g in range(trips * INNER, groups):
                    acc = acc + ref[pl.ds(row0 + g * SUB, SUB), :]
                return acc

            acc = jnp.zeros((SUB, n), jnp.float32)
            for c in range(n_chunks):
                if c == assist_at:
                    for k, cp in enumerate(assists):
                        cp.wait_recv()
                        acc = accumulate(abuf, k * a_rows, a_rows, acc)
                load(c).wait()
                acc = accumulate(xbuf, offs[c], chunks[c], acc)

            row = lax.broadcasted_iota(jnp.int32, (SUB, LANES), 0)
            d_copies = []
            for s in range(n_stairs):
                stair_load(s).wait()
                vs = []
                for j in range(s_off[s], s_off[s + 1]):
                    cols = slice(j * LANES, (j + 1) * LANES)
                    terms = [
                        xbuf[pl.ds(s_row0 + g * SUB, SUB), cols]
                        for g in range(STAIR_ROWS // SUB)
                    ]
                    terms.append(acc[:, cols])
                    while len(terms) > 1:
                        terms = [
                            terms[i] + terms[i + 1] if i + 1 < len(terms) else terms[i]
                            for i in range(0, len(terms), 2)
                        ]
                    vs.append(terms[0])
                shift = 1
                while shift < SUB:
                    if len(vs) > 1:
                        keep = (row & shift) == 0
                        vs = [
                            jnp.where(keep, vs[2 * j], vs[2 * j + 1])
                            + pltpu.roll(
                                jnp.where(keep, vs[2 * j + 1], vs[2 * j]), shift, 0
                            )
                            for j in range(len(vs) // 2)
                        ]
                    else:
                        vs = [vs[0] + pltpu.roll(vs[0], shift, 0)]
                    shift *= 2
                packed = vs[0] * inv_total
                rows = pl.ds(s_off[s], STAIR_BLOCKS[s])
                comm[0, rows, :] = packed[s_off[s] : s_off[s + 1], :]
                cp = pltpu.make_async_remote_copy(
                    src_ref=comm.at[0, rows],
                    dst_ref=comm.at[diag, rows],
                    send_sem=d_send_sems.at[s],
                    recv_sem=d_recv_sem,
                    device_id=peer(diag),
                    device_id_type=pl.DeviceIdType.MESH,
                )
                cp.start()
                d_copies.append(cp)

            n_copies = []
            for k, d in enumerate(nbrs):
                cp = pltpu.make_async_remote_copy(
                    src_ref=comm.at[0],
                    dst_ref=comm.at[d],
                    send_sem=n_send_sems.at[k],
                    recv_sem=n_recv_sems.at[k],
                    device_id=peer(d),
                    device_id_type=pl.DeviceIdType.MESH,
                )
                cp.start()
                n_copies.append(cp)

            total = comm[0]
            for cp in assists + d_copies + n_copies:
                cp.wait_send()
            for cp, d in zip(n_copies, nbrs):
                cp.wait_recv()
                total = total + comm[d]
            pltpu.make_async_copy(comm.at[diag], comm.at[diag], d_recv_sem).wait()
            out_ref[...] = total + comm[diag]

        pl.run_scoped(
            scoped,
            pltpu.SemaphoreType.DMA((n_chunks,)),
            pltpu.SemaphoreType.DMA((n_stairs,)),
            pltpu.SemaphoreType.DMA((2,)),
            pltpu.SemaphoreType.DMA((2,)),
            pltpu.SemaphoreType.DMA((n_stairs,)),
            pltpu.SemaphoreType.DMA,
            pltpu.SemaphoreType.DMA((2,)),
            pltpu.SemaphoreType.DMA((2,)),
        )

    out = pl.pallas_call(
        kernel_body,
        out_shape=jax.ShapeDtypeStruct((nb, LANES), jnp.float32),
        in_specs=[pl.BlockSpec(memory_space=pl.ANY)],
        out_specs=pl.BlockSpec(memory_space=pltpu.VMEM),
        scratch_shapes=[
            pltpu.VMEM((l_rows, n), jnp.float32),
            pltpu.VMEM((2 * a_rows, n), jnp.float32),
            pltpu.VMEM((N_DEV, nb, LANES), jnp.float32),
        ],
        compiler_params=pltpu.CompilerParams(collective_id=0),
    )(x)
    return out.reshape(1, n)
```
